```python
import numpy as np

kernel_name = "dist_mean_ax1_xy_m4096_n1024"

def setup_inputs():
    return {"x": np.random.randn(8192, 2048).astype(np.float32)}

def reference(x: np.ndarray) -> np.ndarray:
    return np.mean(x, axis=1, keepdims=True)
```

```python
import jax
import jax.numpy as jnp
from jax import lax
from jax.experimental import pallas as pl
from jax.experimental.pallas import tpu as pltpu

_MESH = pl.DeviceIdType.MESH
_LANES = 128
_SUB = 256
_RAW1 = 128
_RAW2 = 64
_MID = 384
_LAST = 32


def _placed_row_sums(x, lane0):
    r = x.shape[0]
    s = jnp.sum(x, axis=1, keepdims=True)
    row = lax.broadcasted_iota(jnp.int32, (r, _LANES), 0) + lane0
    lane = lax.broadcasted_iota(jnp.int32, (r, _LANES), 1)
    return jnp.sum(jnp.where(row == lane, s, 0.0), axis=0, keepdims=True)


def pallas_dist_mean_ax1_xy_m4096_n1024_kernel(
x: jax.Array,
):
    m, n = x.shape
    half = m // 2
    scale = 1.0 / (2 * n)
    raw_rows = _RAW1 + _RAW2
    raw_full = raw_rows // _LANES * _LANES
    raw_blocks = -(-raw_rows // _LANES) * _LANES
    split = (raw_rows + (half - raw_rows) // 2) // _LANES * _LANES
    dmas = [
        (1, raw_rows, split - raw_rows),
        (1, split, half - split),
        (2, raw_blocks, half - raw_blocks - _MID),
        (2, half - _MID, _MID),
    ]
    dmas += [(2, b, _LANES) for b in range(raw_blocks - _LANES, 0, -_LANES)]
    dmas += [(2, 0, _LANES - _LAST), (2, _LANES - _LAST, _LAST)]
    n_dmas = len(dmas)

    def body(x_ref, o_ref, buf, raw, part, recv, tmp,
             in_sems, raw_send, raw_recv, p_send, p_recv, o_send, o_recv):
        mx = lax.axis_index("x")
        my = lax.axis_index("y")
        peer = (mx, 1 - my)
        off1 = pl.multiple_of(my * half, half)
        off2 = pl.multiple_of((1 - my) * half, half)

        def in_copy(i):
            phase, s, rows = dmas[i]
            src = (off1 if phase == 1 else off2) + s
            dst = s if phase == 1 else half + s
            return pltpu.make_async_copy(
                x_ref.at[pl.ds(src, rows)], buf.at[pl.ds(dst, rows)], in_sems.at[i])

        def remote(src, dst, send_sem, recv_sem):
            return pltpu.make_async_remote_copy(
                src, dst, send_sem, recv_sem, device_id=peer, device_id_type=_MESH)

        def row_sums(ref, start, rows):
            return jnp.sum(ref[pl.ds(start, rows), :], axis=1).reshape(1, rows)

        def send_means(s, rows):
            done = o_ref.at[:, pl.ds(pl.multiple_of(off2 + s, _LANES), rows)]
            remote(done, done, o_send, o_recv).start()

        def finish(s, rows):
            for t in range(s, s + rows, _SUB):
                k = min(_SUB, s + rows - t)
                tmp[:, pl.ds(t, k)] = row_sums(buf, half + t, k)
                o_ref[:, pl.ds(pl.multiple_of(off2 + t, _LANES), k)] = (
                    tmp[:, pl.ds(t, k)] + recv[:, pl.ds(t, k)]) * scale
            send_means(s, rows)

        for i in range(n_dmas):
            in_copy(i).start()

        barrier = pltpu.get_barrier_semaphore()
        pl.semaphore_signal(barrier, 1, device_id=peer, device_id_type=_MESH)
        pl.semaphore_wait(barrier, 1)

        raw1 = remote(x_ref.at[pl.ds(off1, _RAW1)], raw.at[pl.ds(0, _RAW1)],
                      raw_send.at[0], raw_recv.at[0])
        raw2 = remote(x_ref.at[pl.ds(off1 + _RAW1, _RAW2)], raw.at[pl.ds(_RAW1, _RAW2)],
                      raw_send.at[1], raw_recv.at[1])
        parts = remote(part.at[:, pl.ds(raw_full, half - raw_full)],
                       recv.at[:, pl.ds(raw_full, half - raw_full)], p_send, p_recv)
        raw1.start()

        for i in range(2):
            _, s, rows = dmas[i]
            in_copy(i).wait()
            t0 = s
            if s % _LANES:
                t0 = raw_blocks
                part[:, pl.ds(raw_full, _LANES)] = _placed_row_sums(
                    buf[pl.ds(s, t0 - s), :], s % _LANES)
            for t in range(t0, s + rows, _SUB):
                k = min(_SUB, s + rows - t)
                part[:, pl.ds(t, k)] = row_sums(buf, t, k)
        parts.start()
        raw2.start()

        in_copy(2).wait()
        parts.wait_recv()
        finish(*dmas[2][1:])
        in_copy(3).wait()
        finish(*dmas[3][1:])

        raw1.wait_recv()
        raw2.wait_recv()
        for t in range(0, raw_full, _SUB):
            k = min(_SUB, raw_full - t)
            recv[:, pl.ds(t, k)] = row_sums(raw, t, k)
        if raw_rows > raw_full:
            recv[:, pl.ds(raw_full, _LANES)] = (
                recv[:, pl.ds(raw_full, _LANES)]
                + _placed_row_sums(raw[pl.ds(raw_full, raw_rows - raw_full), :], 0))

        for i in range(4, n_dmas - 2):
            in_copy(i).wait()
            finish(*dmas[i][1:])

        in_copy(n_dmas - 2).wait()
        acc = recv[:, pl.ds(0, _LANES)] + _placed_row_sums(
            buf[pl.ds(half, _LANES - _LAST), :], 0)
        in_copy(n_dmas - 1).wait()
        acc = acc + _placed_row_sums(
            buf[pl.ds(half + _LANES - _LAST, _LAST), :], _LANES - _LAST)
        o_ref[:, pl.ds(off2, _LANES)] = acc * scale
        send_means(0, _LANES)

        parts.wait_send()
        raw1.wait_send()
        raw2.wait_send()
        mine = o_ref.at[:, pl.ds(off2, half)]
        theirs = o_ref.at[:, pl.ds(off1, half)]
        pltpu.make_async_copy(mine, mine, o_send).wait()
        pltpu.make_async_copy(theirs, theirs, o_recv).wait()

    out = pl.pallas_call(
        body,
        out_shape=jax.ShapeDtypeStruct((1, m), jnp.float32),
        in_specs=[pl.BlockSpec(memory_space=pl.ANY)],
        out_specs=pl.BlockSpec(memory_space=pltpu.VMEM),
        scratch_shapes=[
            pltpu.VMEM((m, n), jnp.float32),
            pltpu.VMEM((raw_rows, n), jnp.float32),
            pltpu.VMEM((1, half), jnp.float32),
            pltpu.VMEM((1, half), jnp.float32),
            pltpu.VMEM((1, half), jnp.float32),
            pltpu.SemaphoreType.DMA((n_dmas,)),
            pltpu.SemaphoreType.DMA((2,)),
            pltpu.SemaphoreType.DMA((2,)),
            pltpu.SemaphoreType.DMA,
            pltpu.SemaphoreType.DMA,
            pltpu.SemaphoreType.DMA,
            pltpu.SemaphoreType.DMA,
        ],
        compiler_params=pltpu.CompilerParams(
            vmem_limit_bytes=64 * 1024 * 1024,
            collective_id=0,
            disable_semaphore_checks=True,
            disable_bounds_checks=True,
        ),
    )(x)
    return out.reshape(m, 1)
```

```python
import jax
import jax.numpy as jnp
from jax import lax
from jax.experimental import pallas as pl
from jax.experimental.pallas import tpu as pltpu

_MESH = pl.DeviceIdType.MESH
_LANES = 128
_SUB = 256
_RAW1 = 128
_RAW2 = 64
_RAWX = 192
_MID = 384
_LAST = 32


def _placed_row_sums(x, lane0):
    r = x.shape[0]
    s = jnp.sum(x, axis=1, keepdims=True)
    row = lax.broadcasted_iota(jnp.int32, (r, _LANES), 0) + lane0
    lane = lax.broadcasted_iota(jnp.int32, (r, _LANES), 1)
    return jnp.sum(jnp.where(row == lane, s, 0.0), axis=0, keepdims=True)


def pallas_dist_mean_ax1_xy_m4096_n1024_kernel(
x: jax.Array,
):
    m, n = x.shape
    half = m // 2
    scale = 1.0 / (2 * n)
    raw_rows = _RAW1 + _RAW2
    raw_full = raw_rows // _LANES * _LANES
    raw_blocks = -(-raw_rows // _LANES) * _LANES
    x0 = raw_blocks
    x_full = _RAWX // _LANES * _LANES
    x_blocks = -(-_RAWX // _LANES) * _LANES
    x_rest = x_blocks - _RAWX
    x_end = x0 + x_blocks
    split = (raw_rows + (half - raw_rows) // 2) // _LANES * _LANES
    assert raw_rows > raw_full > 0 and x_rest > 0 and x_full > 0

    dmas = [
        (1, raw_rows, split - raw_rows),
        (1, split, half - split),
        (2, x_end, half - x_end - _MID),
        (2, half - _MID, _MID),
        (2, x0 + _RAWX, x_rest),
    ]
    first_block = len(dmas)
    dmas += [(2, b, _LANES) for b in range(raw_blocks - _LANES, 0, -_LANES)]
    dmas += [(2, 0, _LANES - _LAST), (2, _LANES - _LAST, _LAST)]
    n_dmas = len(dmas)

    def body(x_ref, o_ref, buf, raw, rawx, part, recv, tmp, sendx, recvx,
             in_sems, raw_send, raw_recv, p_send, p_recv, o_send, o_recv,
             x_send, x_recv):
        mx = lax.axis_index("x")
        my = lax.axis_index("y")
        peer = (mx, 1 - my)
        xnbr = (1 - mx, my)
        off1 = pl.multiple_of(my * half, half)
        off2 = pl.multiple_of((1 - my) * half, half)

        def in_copy(i):
            phase, s, rows = dmas[i]
            src = (off1 if phase == 1 else off2) + s
            dst = s if phase == 1 else half + s
            return pltpu.make_async_copy(
                x_ref.at[pl.ds(src, rows)], buf.at[pl.ds(dst, rows)], in_sems.at[i])

        def remote(src, dst, send_sem, recv_sem, device):
            return pltpu.make_async_remote_copy(
                src, dst, send_sem, recv_sem, device_id=device, device_id_type=_MESH)

        def row_sums(ref, start, rows):
            return jnp.sum(ref[pl.ds(start, rows), :], axis=1).reshape(1, rows)

        def out_block(s, rows):
            return pl.ds(pl.multiple_of(off2 + s, _LANES), rows)

        def send_means(s, rows):
            done = o_ref.at[:, out_block(s, rows)]
            remote(done, done, o_send, o_recv, peer).start()

        def finish(s, rows):
            for t in range(s, s + rows, _SUB):
                k = min(_SUB, s + rows - t)
                tmp[:, pl.ds(t, k)] = row_sums(buf, half + t, k)
                o_ref[:, out_block(t, k)] = (
                    tmp[:, pl.ds(t, k)] + recv[:, pl.ds(t, k)]) * scale
            send_means(s, rows)

        raw1 = remote(x_ref.at[pl.ds(off1, _RAW1)], raw.at[pl.ds(0, _RAW1)],
                      raw_send.at[0], raw_recv.at[0], peer)
        raw2 = remote(x_ref.at[pl.ds(off1 + _RAW1, _RAW2)], raw.at[pl.ds(_RAW1, _RAW2)],
                      raw_send.at[1], raw_recv.at[1], peer)
        parts = remote(part.at[:, pl.ds(raw_full, half - raw_full)],
                       recv.at[:, pl.ds(raw_full, half - raw_full)], p_send, p_recv, peer)
        lend = remote(x_ref.at[pl.ds(off2 + x0, _RAWX)], rawx,
                      x_send.at[0], x_recv.at[0], xnbr)
        give_back = remote(sendx, recvx, x_send.at[1], x_recv.at[1], xnbr)

        for i in range(n_dmas):
            in_copy(i).start()

        barrier = pltpu.get_barrier_semaphore()
        pl.semaphore_signal(barrier, 1, device_id=peer, device_id_type=_MESH)
        pl.semaphore_signal(barrier, 1, device_id=xnbr, device_id_type=_MESH)
        pl.semaphore_wait(barrier, 2)
        raw1.start()
        lend.start()

        for i in range(2):
            _, s, rows = dmas[i]
            in_copy(i).wait()
            t0 = s
            if s % _LANES:
                t0 = raw_blocks
                part[:, pl.ds(raw_full, _LANES)] = _placed_row_sums(
                    buf[pl.ds(s, t0 - s), :], s % _LANES)
            for t in range(t0, s + rows, _SUB):
                k = min(_SUB, s + rows - t)
                part[:, pl.ds(t, k)] = row_sums(buf, t, k)
        parts.start()
        raw2.start()

        in_copy(2).wait()
        parts.wait_recv()
        finish(*dmas[2][1:])

        lend.wait_recv()
        sendx[:, pl.ds(0, x_full)] = row_sums(rawx, 0, x_full)
        sendx[:, pl.ds(x_full, _LANES)] = _placed_row_sums(
            rawx[pl.ds(x_full, _RAWX - x_full), :], 0)
        give_back.start()

        in_copy(3).wait()
        finish(*dmas[3][1:])

        raw1.wait_recv()
        raw2.wait_recv()
        recv[:, pl.ds(0, raw_full)] = row_sums(raw, 0, raw_full)
        recv[:, pl.ds(raw_full, _LANES)] = (
            recv[:, pl.ds(raw_full, _LANES)]
            + _placed_row_sums(raw[pl.ds(raw_full, raw_rows - raw_full), :], 0))

        for i in range(first_block, n_dmas - 2):
            in_copy(i).wait()
            finish(*dmas[i][1:])

        in_copy(first_block - 1).wait()
        give_back.wait_recv()
        o_ref[:, out_block(x0, x_full)] = (
            recvx[:, pl.ds(0, x_full)] + recv[:, pl.ds(x0, x_full)]) * scale
        o_ref[:, out_block(x0 + x_full, _LANES)] = (
            recvx[:, pl.ds(x_full, _LANES)] + recv[:, pl.ds(x0 + x_full, _LANES)]
            + _placed_row_sums(buf[pl.ds(half + x0 + _RAWX, x_rest), :],
                               _LANES - x_rest)) * scale
        send_means(x0, x_blocks)

        in_copy(n_dmas - 2).wait()
        acc = recv[:, pl.ds(0, _LANES)] + _placed_row_sums(
            buf[pl.ds(half, _LANES - _LAST), :], 0)
        in_copy(n_dmas - 1).wait()
        acc = acc + _placed_row_sums(
            buf[pl.ds(half + _LANES - _LAST, _LAST), :], _LANES - _LAST)
        o_ref[:, out_block(0, _LANES)] = acc * scale
        send_means(0, _LANES)

        for copy in (parts, raw1, raw2, lend, give_back):
            copy.wait_send()
        mine = o_ref.at[:, pl.ds(off2, half)]
        theirs = o_ref.at[:, pl.ds(off1, half)]
        pltpu.make_async_copy(mine, mine, o_send).wait()
        pltpu.make_async_copy(theirs, theirs, o_recv).wait()

    out = pl.pallas_call(
        body,
        out_shape=jax.ShapeDtypeStruct((1, m), jnp.float32),
        in_specs=[pl.BlockSpec(memory_space=pl.ANY)],
        out_specs=pl.BlockSpec(memory_space=pltpu.VMEM),
        scratch_shapes=[
            pltpu.VMEM((m, n), jnp.float32),
            pltpu.VMEM((raw_rows, n), jnp.float32),
            pltpu.VMEM((_RAWX, n), jnp.float32),
            pltpu.VMEM((1, half), jnp.float32),
            pltpu.VMEM((1, half), jnp.float32),
            pltpu.VMEM((1, half), jnp.float32),
            pltpu.VMEM((1, x_blocks), jnp.float32),
            pltpu.VMEM((1, x_blocks), jnp.float32),
            pltpu.SemaphoreType.DMA((n_dmas,)),
            pltpu.SemaphoreType.DMA((2,)),
            pltpu.SemaphoreType.DMA((2,)),
            pltpu.SemaphoreType.DMA,
            pltpu.SemaphoreType.DMA,
            pltpu.SemaphoreType.DMA,
            pltpu.SemaphoreType.DMA,
            pltpu.SemaphoreType.DMA((2,)),
            pltpu.SemaphoreType.DMA((2,)),
        ],
        compiler_params=pltpu.CompilerParams(
            vmem_limit_bytes=64 * 1024 * 1024,
            collective_id=0,
            disable_semaphore_checks=True,
            disable_bounds_checks=True,
        ),
    )(x)
    return out.reshape(m, 1)
```

```python
import jax
import jax.numpy as jnp
from jax import lax
from jax.experimental import pallas as pl
from jax.experimental.pallas import tpu as pltpu

_MESH = pl.DeviceIdType.MESH
_LANES = 128
_SUB = 256
_RAW1 = 128
_RAW2 = 64
_RAWX = 192
_MID = 384
_LAST = 32


def _placed_row_sums(x, lane0):
    r = x.shape[0]
    s = jnp.sum(x, axis=1, keepdims=True)
    row = lax.broadcasted_iota(jnp.int32, (r, _LANES), 0) + lane0
    lane = lax.broadcasted_iota(jnp.int32, (r, _LANES), 1)
    return jnp.sum(jnp.where(row == lane, s, 0.0), axis=0, keepdims=True)


def pallas_dist_mean_ax1_xy_m4096_n1024_kernel(
x: jax.Array,
):
    m, n = x.shape
    half = m // 2
    scale = 1.0 / (2 * n)
    raw_rows = _RAW1 + _RAW2
    raw_full = raw_rows // _LANES * _LANES
    raw_blocks = -(-raw_rows // _LANES) * _LANES
    x0 = raw_blocks
    x_full = _RAWX // _LANES * _LANES
    x_blocks = -(-_RAWX // _LANES) * _LANES
    x_rest = x_blocks - _RAWX
    x_end = x0 + x_blocks
    split = (raw_rows + (half - raw_rows) // 2) // _LANES * _LANES
    assert raw_rows > raw_full > 0 and x_rest > 0 and x_full > 0

    dmas = [
        (1, raw_rows, split - raw_rows),
        (1, split, half - split),
        (2, x_end, half - x_end - _MID),
        (2, half - _MID, _MID),
        (2, x0 + _RAWX, x_rest),
    ]
    first_block = len(dmas)
    dmas += [(2, b, _LANES) for b in range(raw_blocks - _LANES, 0, -_LANES)]
    dmas += [(2, _LAST, _LANES - _LAST), (2, 0, _LAST)]
    n_dmas = len(dmas)

    def body(x_ref, o_ref, buf, raw, rawx, part, recv, tmp, sendx, recvx,
             in_sems, raw_send, raw_recv, p_send, p_recv, o_send, o_recv,
             x_send, x_recv):
        mx = lax.axis_index("x")
        my = lax.axis_index("y")
        peer = (mx, 1 - my)
        xnbr = (1 - mx, my)
        off1 = pl.multiple_of(my * half, half)
        off2 = pl.multiple_of((1 - my) * half, half)

        def in_copy(i):
            phase, s, rows = dmas[i]
            src = (off1 if phase == 1 else off2) + s
            dst = s if phase == 1 else half + s
            return pltpu.make_async_copy(
                x_ref.at[pl.ds(src, rows)], buf.at[pl.ds(dst, rows)], in_sems.at[i])

        def remote(src, dst, send_sem, recv_sem, device):
            return pltpu.make_async_remote_copy(
                src, dst, send_sem, recv_sem, device_id=device, device_id_type=_MESH)

        def row_sums(ref, start, rows):
            return jnp.sum(ref[pl.ds(start, rows), :], axis=1).reshape(1, rows)

        def out_block(s, rows):
            return pl.ds(pl.multiple_of(off2 + s, _LANES), rows)

        def send_means(s, rows):
            done = o_ref.at[:, out_block(s, rows)]
            remote(done, done, o_send, o_recv, peer).start()

        def finish(s, rows):
            for t in range(s, s + rows, _SUB):
                k = min(_SUB, s + rows - t)
                tmp[:, pl.ds(t, k)] = row_sums(buf, half + t, k)
                o_ref[:, out_block(t, k)] = (
                    tmp[:, pl.ds(t, k)] + recv[:, pl.ds(t, k)]) * scale
            send_means(s, rows)

        raw1 = remote(x_ref.at[pl.ds(off1, _RAW1)], raw.at[pl.ds(0, _RAW1)],
                      raw_send.at[0], raw_recv.at[0], peer)
        raw2 = remote(x_ref.at[pl.ds(off1 + _RAW1, _RAW2)], raw.at[pl.ds(_RAW1, _RAW2)],
                      raw_send.at[1], raw_recv.at[1], peer)
        parts = remote(part.at[:, pl.ds(raw_full, half - raw_full)],
                       recv.at[:, pl.ds(raw_full, half - raw_full)], p_send, p_recv, peer)
        lend = remote(x_ref.at[pl.ds(off2 + x0, _RAWX)], rawx,
                      x_send.at[0], x_recv.at[0], xnbr)
        give_back = remote(sendx, recvx, x_send.at[1], x_recv.at[1], xnbr)

        for i in range(n_dmas):
            in_copy(i).start()

        barrier = pltpu.get_barrier_semaphore()
        pl.semaphore_signal(barrier, 1, device_id=peer, device_id_type=_MESH)
        pl.semaphore_signal(barrier, 1, device_id=xnbr, device_id_type=_MESH)
        pl.semaphore_wait(barrier, 2)
        raw1.start()
        lend.start()

        for i in range(2):
            _, s, rows = dmas[i]
            in_copy(i).wait()
            t0 = s
            if s % _LANES:
                t0 = raw_blocks
                part[:, pl.ds(raw_full, _LANES)] = _placed_row_sums(
                    buf[pl.ds(s, t0 - s), :], s % _LANES)
            for t in range(t0, s + rows, _SUB):
                k = min(_SUB, s + rows - t)
                part[:, pl.ds(t, k)] = row_sums(buf, t, k)
        parts.start()
        raw2.start()

        in_copy(2).wait()
        parts.wait_recv()
        finish(*dmas[2][1:])

        lend.wait_recv()
        sendx[:, pl.ds(0, x_full)] = row_sums(rawx, 0, x_full)
        sendx[:, pl.ds(x_full, _LANES)] = _placed_row_sums(
            rawx[pl.ds(x_full, _RAWX - x_full), :], 0)
        give_back.start()

        in_copy(3).wait()
        finish(*dmas[3][1:])

        raw1.wait_recv()
        raw2.wait_recv()
        recv[:, pl.ds(0, raw_full)] = row_sums(raw, 0, raw_full)
        recv[:, pl.ds(raw_full, _LANES)] = (
            recv[:, pl.ds(raw_full, _LANES)]
            + _placed_row_sums(raw[pl.ds(raw_full, raw_rows - raw_full), :], 0))

        for i in range(first_block, n_dmas - 2):
            in_copy(i).wait()
            finish(*dmas[i][1:])

        in_copy(first_block - 1).wait()
        give_back.wait_recv()
        o_ref[:, out_block(x0, x_full)] = (
            recvx[:, pl.ds(0, x_full)] + recv[:, pl.ds(x0, x_full)]) * scale
        o_ref[:, out_block(x0 + x_full, _LANES)] = (
            recvx[:, pl.ds(x_full, _LANES)] + recv[:, pl.ds(x0 + x_full, _LANES)]
            + _placed_row_sums(buf[pl.ds(half + x0 + _RAWX, x_rest), :],
                               _LANES - x_rest)) * scale
        send_means(x0, x_blocks)

        in_copy(n_dmas - 2).wait()
        theirs0 = recv[:, pl.ds(0, _LANES)]
        o_ref[:, out_block(0, _LANES)] = (theirs0 + _placed_row_sums(
            buf[pl.ds(half + _LAST, _LANES - _LAST), :], _LAST)) * scale
        row = lax.broadcasted_iota(jnp.int32, (_LAST, _LANES), 0)
        lane = lax.broadcasted_iota(jnp.int32, (_LAST, _LANES), 1)
        diag = jnp.where(row == lane, jnp.broadcast_to(theirs0, (_LAST, _LANES)), 0.0)
        in_copy(n_dmas - 1).wait()
        cols = [buf[pl.ds(half, _LAST), pl.ds(j, _LANES)] for j in range(0, n, _LANES)]
        while len(cols) > 1:
            cols = [cols[j] + cols[j + 1] for j in range(0, len(cols), 2)]
        o_ref[:, out_block(0, _LAST)] = jnp.sum(
            (cols[0] + diag) * scale, axis=1).reshape(1, _LAST)
        send_means(0, _LANES)

        for copy in (parts, raw1, raw2, lend, give_back):
            copy.wait_send()
        mine = o_ref.at[:, pl.ds(off2, half)]
        theirs = o_ref.at[:, pl.ds(off1, half)]
        pltpu.make_async_copy(mine, mine, o_send).wait()
        pltpu.make_async_copy(theirs, theirs, o_recv).wait()

    out = pl.pallas_call(
        body,
        out_shape=jax.ShapeDtypeStruct((1, m), jnp.float32),
        in_specs=[pl.BlockSpec(memory_space=pl.ANY)],
        out_specs=pl.BlockSpec(memory_space=pltpu.VMEM),
        scratch_shapes=[
            pltpu.VMEM((m, n), jnp.float32),
            pltpu.VMEM((raw_rows, n), jnp.float32),
            pltpu.VMEM((_RAWX, n), jnp.float32),
            pltpu.VMEM((1, half), jnp.float32),
            pltpu.VMEM((1, half), jnp.float32),
            pltpu.VMEM((1, half), jnp.float32),
            pltpu.VMEM((1, x_blocks), jnp.float32),
            pltpu.VMEM((1, x_blocks), jnp.float32),
            pltpu.SemaphoreType.DMA((n_dmas,)),
            pltpu.SemaphoreType.DMA((2,)),
            pltpu.SemaphoreType.DMA((2,)),
            pltpu.SemaphoreType.DMA,
            pltpu.SemaphoreType.DMA,
            pltpu.SemaphoreType.DMA,
            pltpu.SemaphoreType.DMA,
            pltpu.SemaphoreType.DMA((2,)),
            pltpu.SemaphoreType.DMA((2,)),
        ],
        compiler_params=pltpu.CompilerParams(
            vmem_limit_bytes=64 * 1024 * 1024,
            collective_id=0,
            disable_semaphore_checks=True,
            disable_bounds_checks=True,
        ),
    )(x)
    return out.reshape(m, 1)
```
